```python
import numpy as np

kernel_name = "dist_mean_ax1_xy_m1024_n512"

def setup_inputs():
    return {"x": np.random.randn(2048, 1024).astype(np.float32)}

def reference(x: np.ndarray) -> np.ndarray:
    return np.mean(x, axis=1, keepdims=True)
```

```python
import jax
import jax.numpy as jnp
from jax import lax
from jax.experimental import pallas as pl
from jax.experimental.pallas import tpu as pltpu

LANES = 128
SUB = 8

LATE_BOUNDS = (0, 256, 512, 768, 872, 920, 960, 968)
EARLY_BOUNDS = (0, 256, 512, 768, 1024)
LATE_SENDS = ((2, 0, 6), (5, 6, 7), (6, 7, 8))
EARLY_SENDS = ((3, 0, 8),)
LATE_REDUCE_WITH = {5: 6}
LATE_FLUSH_AT = {6: 5}


def pallas_dist_mean_ax1_xy_m1024_n512_kernel(x: jax.Array):
    m, n = x.shape
    scale = 1.0 / (2 * n)
    main = LATE_BOUNDS[-1]
    raw = m - main
    assert EARLY_BOUNDS[-1] == m and LATE_BOUNDS[1] == EARLY_BOUNDS[1]
    assert n % LANES == 0 and (n // LANES) & (n // LANES - 1) == 0

    def tiles_of(rows, r0):
        parts = [rows[:, k * LANES:(k + 1) * LANES] for k in range(n // LANES)]
        while len(parts) > 1:
            parts = [parts[i] + parts[i + 1] for i in range(0, len(parts), 2)]
        p = parts[0]
        return {r0 + SUB * k: p[SUB * k:SUB * (k + 1)] for k in range(p.shape[0] // SUB)}

    def scatter(g, tile, acc):
        diff = (lax.broadcasted_iota(jnp.int32, (SUB, LANES), 1)
                - lax.broadcasted_iota(jnp.int32, (SUB, LANES), 0))
        s = jnp.sum(tile, axis=1, keepdims=True)
        b = g // LANES
        prev = acc[b] if b in acc else jnp.zeros((SUB, LANES), jnp.float32)
        acc[b] = jnp.where(diff == g % LANES, s, prev)

    def block(b):
        return pl.ds(b * LANES, LANES)

    def body(x_hbm, out_ref, xbuf, rawbuf, send_buf, recv_buf, in_sems,
             late_ssem, late_rsem, early_ssem, early_rsem, raw_ssem, raw_rsem):
        def load(c, lo, hi):
            return pltpu.make_async_copy(
                x_hbm.at[pl.ds(lo, hi - lo)], xbuf.at[pl.ds(lo, hi - lo)], in_sems.at[c])

        first = load(0, 0, LATE_BOUNDS[1])
        first.start()

        my_x = lax.axis_index("x")
        my_y = lax.axis_index("y")
        peer = (my_x, 1 - my_y)

        def sums_rdma(g, blo, bhi, ssem, rsem):
            sl = pl.ds(blo * LANES, (bhi - blo) * LANES)
            return pltpu.make_async_remote_copy(
                src_ref=send_buf.at[:, sl], dst_ref=recv_buf.at[:, sl],
                send_sem=ssem.at[g], recv_sem=rsem.at[g],
                device_id=peer, device_id_type=pl.DeviceIdType.MESH)

        raw_rdma = pltpu.make_async_remote_copy(
            src_ref=x_hbm.at[pl.ds(main, raw)], dst_ref=rawbuf,
            send_sem=raw_ssem, recv_sem=raw_rsem,
            device_id=peer, device_id_type=pl.DeviceIdType.MESH)
        late_rdmas = [sums_rdma(g, lo, hi, late_ssem, late_rsem)
                      for g, (_, lo, hi) in enumerate(LATE_SENDS)]
        early_rdmas = [sums_rdma(g, lo, hi, early_ssem, early_rsem)
                       for g, (_, lo, hi) in enumerate(EARLY_SENDS)]

        barrier = pltpu.get_barrier_semaphore()
        pl.semaphore_signal(barrier, inc=1, device_id=peer,
                            device_id_type=pl.DeviceIdType.MESH)

        def start_loads(bounds):
            loads = [first]
            for c in range(1, len(bounds) - 1):
                loads.append(load(c, bounds[c], bounds[c + 1]))
                loads[-1].start()
            return loads

        def reduce_and_send(bounds, loads, sends, rdmas, reduce_with, flush_at,
                            before_first_send):
            acc, tiles = {}, {}
            left = {}
            for g in range(0, bounds[-1], SUB):
                left[g // LANES] = left.get(g // LANES, 0) + 1
            for c in range(len(bounds) - 1):
                lo, hi = bounds[c], bounds[c + 1]
                loads[c].wait()
                tiles.update(tiles_of(xbuf[pl.ds(lo, hi - lo), :], lo))
                if reduce_with.get(c, c) == c:
                    for g in sorted(tiles, key=lambda g: (g // LANES in flush_at, g)):
                        scatter(g, tiles[g], acc)
                        left[g // LANES] -= 1
                    tiles = {}
                for b in [b for b in acc if left[b] == 0 and flush_at.get(b, c) <= c]:
                    send_buf[:, block(b)] = jnp.sum(acc.pop(b), axis=0, keepdims=True)
                for g, (cc, blo, bhi) in enumerate(sends):
                    if cc == c:
                        assert all(left[b] == 0 and b not in acc for b in range(blo, bhi))
                        if g == 0 and before_first_send is not None:
                            before_first_send()
                        rdmas[g].start()

        def raw_sums(rows):
            acc = {}
            for g, tile in tiles_of(rows, main).items():
                scatter(g, tile, acc)
            return {b: jnp.sum(a, axis=0, keepdims=True) for b, a in acc.items()}

        def finish(sends, rdmas, extra):
            for g, (_, blo, bhi) in enumerate(sends):
                own = {}
                for b in range(blo, bhi):
                    v = send_buf[:, block(b)]
                    own[b] = v + extra[b] if b in extra else v
                rdmas[g].wait_recv()
                for b, v in own.items():
                    out_ref[:, block(b)] = (v + recv_buf[:, block(b)]) * scale

        @pl.when(my_y == 1)
        def _():
            loads = start_loads(LATE_BOUNDS)
            pl.semaphore_wait(barrier, 1)
            raw_rdma.start()
            reduce_and_send(LATE_BOUNDS, loads, LATE_SENDS, late_rdmas,
                            LATE_REDUCE_WITH, LATE_FLUSH_AT, None)
            tail = load(len(LATE_BOUNDS) - 1, main, m)
            tail.start()
            tail.wait()
            finish(EARLY_SENDS, early_rdmas, raw_sums(xbuf[pl.ds(main, raw), :]))
            for rdma in late_rdmas:
                rdma.wait_send()
            raw_rdma.wait_send()

        @pl.when(my_y == 0)
        def _():
            loads = start_loads(EARLY_BOUNDS)
            reduce_and_send(EARLY_BOUNDS, loads, EARLY_SENDS, early_rdmas, {}, {},
                            lambda: pl.semaphore_wait(barrier, 1))
            for rdma in early_rdmas:
                rdma.wait_send()
            raw_rdma.wait_recv()
            finish(LATE_SENDS, late_rdmas, raw_sums(rawbuf[...]))

    out = pl.pallas_call(
        body,
        out_shape=jax.ShapeDtypeStruct((1, m), jnp.float32),
        in_specs=[pl.BlockSpec(memory_space=pl.ANY)],
        out_specs=pl.BlockSpec(memory_space=pltpu.VMEM),
        scratch_shapes=[
            pltpu.VMEM((m, n), jnp.float32),
            pltpu.VMEM((raw, n), jnp.float32),
            pltpu.VMEM((1, m), jnp.float32),
            pltpu.VMEM((1, m), jnp.float32),
            pltpu.SemaphoreType.DMA((max(len(LATE_BOUNDS), len(EARLY_BOUNDS) - 1),)),
            pltpu.SemaphoreType.DMA((len(LATE_SENDS),)),
            pltpu.SemaphoreType.DMA((len(LATE_SENDS),)),
            pltpu.SemaphoreType.DMA((len(EARLY_SENDS),)),
            pltpu.SemaphoreType.DMA((len(EARLY_SENDS),)),
            pltpu.SemaphoreType.DMA,
            pltpu.SemaphoreType.DMA,
        ],
        compiler_params=pltpu.CompilerParams(
            collective_id=0,
            disable_semaphore_checks=True,
        ),
    )(x)
    return out.reshape(m, 1)
```
